```python
import numpy as np

kernel_name = "dist_rope_attn_htp_bs_b2_sq512_d1024_hq8_dh128"

def setup_inputs():
    x = np.random.randn(8, 512, 1024).astype(np.float32)
    Wq = np.random.randn(1024, 4096).astype(np.float32) * 0.02
    Wk = np.random.randn(1024, 4096).astype(np.float32) * 0.02
    Wv = np.random.randn(1024, 4096).astype(np.float32) * 0.02
    Wo = np.random.randn(4096, 1024).astype(np.float32) * 0.02
    return {"x": x, "Wq": Wq, "Wk": Wk, "Wv": Wv, "Wo": Wo}

def reference(x, Wq, Wk, Wv, Wo):
    B, Sq, Hq, Dh = 8, 512, 32, 128
    inv = 1.0 / (10000.0 ** (np.arange(0, Dh, 2) / Dh))
    pos = np.arange(Sq)[:, None] * inv[None, :]
    cos = np.repeat(np.cos(pos), 2, axis=-1).astype(np.float32)
    sin = np.repeat(np.sin(pos), 2, axis=-1).astype(np.float32)
    def rot(t):
        t2 = t.reshape(B, Sq, Hq, Dh // 2, 2)
        t_r = np.stack([-t2[..., 1], t2[..., 0]], axis=-1).reshape(B, Sq, Hq, Dh)
        return t * cos[None, :, None, :] + t_r * sin[None, :, None, :]
    Q = rot((x @ Wq).reshape(B, Sq, Hq, Dh))
    K = rot((x @ Wk).reshape(B, Sq, Hq, Dh))
    V = (x @ Wv).reshape(B, Sq, Hq, Dh)
    s = np.einsum('bihd,bjhd->bhij', Q, K).astype(np.float32) * 0.08838834764831843
    s_max = s.max(axis=-1, keepdims=True)
    w = np.exp(s - s_max)
    w = w / w.sum(axis=-1, keepdims=True)
    ctx = np.einsum('bhij,bjhd->bihd', w, V).reshape(B, Sq, Hq * Dh)
    return ctx @ Wo
```

```python
import math

import jax
import jax.numpy as jnp
from jax import lax
from jax.experimental import pallas as pl
from jax.experimental.pallas import tpu as pltpu

N_DEV = 4
B_LOC = 2
SQ = 512
D = 1024
HQ = 8
DH = 128
SCALE = 0.08838834764831843


def pallas_dist_rope_attn_htp_bs_b2_sq512_d1024_hq8_dh128_kernel(
    x: jax.Array,
    Wq: jax.Array,
    Wk: jax.Array,
    Wv: jax.Array,
    Wo: jax.Array,
):
    f32 = jnp.float32
    bf16 = jnp.bfloat16

    def body(x_hbm, wq_hbm, wk_hbm, wv_hbm, wo_hbm, out_hbm,
             xin, w32, wqkv, wo, xg, osend, orecv, oacc, ctx, tab,
             ld_sems, st_sems, xs_sems, xr_sems, os_sems, or_sems):
        me = lax.axis_index("i")

        cp_x = pltpu.make_async_copy(x_hbm, xin, ld_sems.at[0])
        cp_x.start()
        w_cps = []
        for i, w_hbm in enumerate((wq_hbm, wk_hbm, wv_hbm, wo_hbm)):
            cp = pltpu.make_async_copy(w_hbm, w32.at[i], ld_sems.at[1 + i])
            cp.start()
            w_cps.append(cp)

        def x_send(d, b):
            r = (N_DEV - d) % N_DEV
            return pltpu.make_async_remote_copy(
                src_ref=xg.at[b],
                dst_ref=xg.at[r * 2 + b],
                send_sem=xs_sems.at[(d - 1) * 2 + b],
                recv_sem=xr_sems.at[(r - 1) * 2 + b],
                device_id=((me + d) % N_DEV,),
                device_id_type=pl.DeviceIdType.MESH,
            )

        cp_x.wait()
        for b in range(B_LOC):
            xg[b] = xin[b].astype(bf16)
            x_send(1, b).start()
            x_send(3, b).start()

        lane = lax.broadcasted_iota(jnp.int32, (SQ, DH), 1)
        pos = lax.broadcasted_iota(jnp.int32, (SQ, DH), 0).astype(f32)
        pair = (lane // 2).astype(f32)
        inv = jnp.exp(pair * (-2.0 * math.log(10000.0) / DH))
        ang = pos * inv
        cos = jnp.cos(ang)
        sin = jnp.sin(ang)
        even = (lane % 2) == 0
        sin_s = jnp.where(even, -sin, sin)
        tab[0] = cos * SCALE
        tab[1] = sin_s * SCALE
        tab[2] = cos
        tab[3] = sin_s

        for i in range(3):
            w_cps[i].wait()
            wqkv[:, i * D:(i + 1) * D] = w32[i].astype(bf16)
        w_cps[3].wait()
        wo[...] = w32[3].astype(bf16)

        def rope(t, c, s):
            a = pltpu.roll(t, DH - 1, 1)
            b_ = pltpu.roll(t, 1, 1)
            ev = (lax.broadcasted_iota(jnp.int32, (SQ, DH), 1) % 2) == 0
            return t * c + jnp.where(ev, a, b_) * s

        def compute(slot):
            xb = xg[slot]
            qkv = jnp.dot(xb, wqkv[...], preferred_element_type=f32)
            for h in range(HQ):
                q = rope(qkv[:, h * DH:(h + 1) * DH], tab[0], tab[1]).astype(bf16)
                k = rope(qkv[:, D + h * DH:D + (h + 1) * DH], tab[2], tab[3]).astype(bf16)
                v = qkv[:, 2 * D + h * DH:2 * D + (h + 1) * DH].astype(bf16)
                s = lax.dot_general(q, k, (((1,), (1,)), ((), ())),
                                    preferred_element_type=f32)
                m = jnp.max(s, axis=-1, keepdims=True)
                p = jnp.exp(s - m)
                l = jnp.sum(p, axis=-1, keepdims=True)
                c = jnp.dot(p.astype(bf16), v, preferred_element_type=f32)
                ctx[:, h * DH:(h + 1) * DH] = (c / l).astype(bf16)
            return jnp.dot(ctx[...], wo[...], preferred_element_type=f32)

        def o_copy(r, b):
            rr = (N_DEV - r) % N_DEV
            return pltpu.make_async_remote_copy(
                src_ref=osend.at[(r - 1) * 2 + b],
                dst_ref=orecv.at[(rr - 1) * 2 + b],
                send_sem=os_sems.at[(r - 1) * 2 + b],
                recv_sem=or_sems.at[(rr - 1) * 2 + b],
                device_id=((me + r) % N_DEV,),
                device_id_type=pl.DeviceIdType.MESH,
            )

        def step(s, carry):
            b = (s >= 4).astype(jnp.int32)
            r = jnp.where((s == 1) | (s == 5), 1,
                          jnp.where((s == 2) | (s == 6), 3,
                                    jnp.where((s == 3) | (s == 4), 2, 0)))
            slot = r * 2 + b

            @pl.when(r > 0)
            def _():
                pltpu.make_async_remote_copy(
                    src_ref=xg.at[slot], dst_ref=xg.at[slot],
                    send_sem=xs_sems.at[0],
                    recv_sem=xr_sems.at[(r - 1) * 2 + b],
                    device_id=(me,), device_id_type=pl.DeviceIdType.MESH,
                ).wait_recv()

            part = compute(slot)

            @pl.when(r == 0)
            def _():
                oacc[b] = part

            @pl.when(r > 0)
            def _():
                osend[(r - 1) * 2 + b] = part.astype(bf16)
                o_copy(r, b).start()

            @pl.when(s == 0)
            def _():
                x_send(2, 0).start()
                x_send(2, 1).start()

            return carry

        lax.fori_loop(0, 8, step, 0)

        for b in range(B_LOC):
            acc = oacc[b]
            for r in range(1, N_DEV):
                idx = (r - 1) * 2 + b
                pltpu.make_async_remote_copy(
                    src_ref=orecv.at[idx], dst_ref=orecv.at[idx],
                    send_sem=os_sems.at[0], recv_sem=or_sems.at[idx],
                    device_id=(me,), device_id_type=pl.DeviceIdType.MESH,
                ).wait_recv()
                acc = acc + orecv[idx].astype(f32)
            oacc[b] = acc
            pltpu.make_async_copy(oacc.at[b], out_hbm.at[b], st_sems.at[b]).start()
        for b in range(B_LOC):
            pltpu.make_async_copy(oacc.at[b], out_hbm.at[b], st_sems.at[b]).wait()
        for d in range(1, N_DEV):
            for b in range(B_LOC):
                x_send(d, b).wait_send()
                o_copy(d, b).wait_send()

    out_shape = jax.ShapeDtypeStruct((B_LOC, SQ, D), jnp.float32)
    any_spec = pl.BlockSpec(memory_space=pl.ANY)
    return pl.pallas_call(
        body,
        out_shape=out_shape,
        in_specs=[any_spec] * 5,
        out_specs=any_spec,
        scratch_shapes=[
            pltpu.VMEM((B_LOC, SQ, D), f32),
            pltpu.VMEM((4, D, D), f32),
            pltpu.VMEM((D, 3 * D), bf16),
            pltpu.VMEM((D, D), bf16),
            pltpu.VMEM((8, SQ, D), bf16),
            pltpu.VMEM((6, SQ, D), bf16),
            pltpu.VMEM((6, SQ, D), bf16),
            pltpu.VMEM((B_LOC, SQ, D), f32),
            pltpu.VMEM((SQ, D), bf16),
            pltpu.VMEM((4, SQ, DH), f32),
            pltpu.SemaphoreType.DMA((5,)),
            pltpu.SemaphoreType.DMA((2,)),
            pltpu.SemaphoreType.DMA((6,)),
            pltpu.SemaphoreType.DMA((6,)),
            pltpu.SemaphoreType.DMA((6,)),
            pltpu.SemaphoreType.DMA((6,)),
        ],
        compiler_params=pltpu.CompilerParams(
            vmem_limit_bytes=100 * 1024 * 1024,
        ),
    )(x, Wq, Wk, Wv, Wo)
```

```python
import math

import jax
import jax.numpy as jnp
from jax import lax
from jax.experimental import pallas as pl
from jax.experimental.pallas import tpu as pltpu

N_DEV = 4
B_LOC = 2
SQ = 512
D = 1024
HQ = 8
DH = 128
SCALE = 0.08838834764831843


def pallas_dist_rope_attn_htp_bs_b2_sq512_d1024_hq8_dh128_kernel(
    x: jax.Array,
    Wq: jax.Array,
    Wk: jax.Array,
    Wv: jax.Array,
    Wo: jax.Array,
):
    f32 = jnp.float32
    bf16 = jnp.bfloat16

    NCH = 12
    CW = 3 * D // NCH

    def body(x_hbm, wq_hbm, wk_hbm, wv_hbm, wo_hbm, out_hbm,
             xin, w32, wqkv, wo, xg, osend, orecv, oacc, ctx, tab,
             ld_sems, st_sems, xs_sems, xr_sems, os_sems, or_sems):
        me = lax.axis_index("i")
        w_hbms = (wq_hbm, wk_hbm, wv_hbm)

        def x_load(b):
            return pltpu.make_async_copy(x_hbm.at[b], xin.at[b], ld_sems.at[b])

        def w_load(j):
            i, c = divmod(j, D // CW)
            return pltpu.make_async_copy(
                w_hbms[i].at[:, pl.ds(c * CW, CW)],
                w32.at[i, :, pl.ds(c * CW, CW)],
                ld_sems.at[2 + j])

        def wo_load(c):
            return pltpu.make_async_copy(
                wo_hbm.at[pl.ds(c * CW, CW), :],
                w32.at[3, pl.ds(c * CW, CW), :],
                ld_sems.at[2 + NCH + c])

        x_load(0).start()
        order = []
        for c in range(D // CW):
            order += [w_load(i * (D // CW) + c) for i in range(3)] + [wo_load(c)]
        for cp in order[:2]:
            cp.start()

        def x_send(d, b):
            r = (N_DEV - d) % N_DEV
            return pltpu.make_async_remote_copy(
                src_ref=xg.at[b],
                dst_ref=xg.at[r * 2 + b],
                send_sem=xs_sems.at[(d - 1) * 2 + b],
                recv_sem=xr_sems.at[(r - 1) * 2 + b],
                device_id=((me + d) % N_DEV,),
                device_id_type=pl.DeviceIdType.MESH,
            )

        lane = lax.broadcasted_iota(jnp.int32, (SQ, DH), 1)
        pos = lax.broadcasted_iota(jnp.int32, (SQ, DH), 0).astype(f32)
        pair = (lane // 2).astype(f32)
        inv = jnp.exp(pair * (-2.0 * math.log(10000.0) / DH))
        ang = pos * inv
        cos = jnp.cos(ang)
        sin = jnp.sin(ang)
        even = (lane % 2) == 0
        sin_s = jnp.where(even, -sin, sin)
        tab[0] = cos * SCALE
        tab[1] = sin_s * SCALE
        tab[2] = cos
        tab[3] = sin_s

        x_load(0).wait()
        xg[0] = xin[0].astype(bf16)
        x_send(1, 0).start()
        x_send(3, 0).start()
        for cp in order[2:]:
            cp.start()
        x_load(1).start()

        def rope(t, c, s):
            a = pltpu.roll(t, DH - 1, 1)
            b_ = pltpu.roll(t, 1, 1)
            ev = (lax.broadcasted_iota(jnp.int32, (SQ, DH), 1) % 2) == 0
            return t * c + jnp.where(ev, a, b_) * s

        def attn_head(q, k, v):
            s = lax.dot_general(q, k, (((1,), (1,)), ((), ())),
                                preferred_element_type=f32)
            m = jnp.max(s, axis=-1, keepdims=True)
            p = jnp.exp(s - m)
            l = jnp.sum(p, axis=-1, keepdims=True)
            c = jnp.dot(p.astype(bf16), v, preferred_element_type=f32)
            return (c / l).astype(bf16)

        def compute(slot):
            qkv = jnp.dot(xg[slot], wqkv[...], preferred_element_type=f32)
            for h in range(HQ):
                q = rope(qkv[:, h * DH:(h + 1) * DH], tab[0], tab[1]).astype(bf16)
                k = rope(qkv[:, D + h * DH:D + (h + 1) * DH],
                         tab[2], tab[3]).astype(bf16)
                v = qkv[:, 2 * D + h * DH:2 * D + (h + 1) * DH].astype(bf16)
                ctx[:, h * DH:(h + 1) * DH] = attn_head(q, k, v)
            return jnp.dot(ctx[...], wo[...], preferred_element_type=f32)

        def o_copy(r, b):
            rr = (N_DEV - r) % N_DEV
            return pltpu.make_async_remote_copy(
                src_ref=osend.at[(r - 1) * 2 + b],
                dst_ref=orecv.at[(rr - 1) * 2 + b],
                send_sem=os_sems.at[(r - 1) * 2 + b],
                recv_sem=or_sems.at[(rr - 1) * 2 + b],
                device_id=((me + r) % N_DEV,),
                device_id_type=pl.DeviceIdType.MESH,
            )

        def finalize(b, acc):
            for r in range(1, N_DEV):
                idx = (r - 1) * 2 + b
                pltpu.make_async_remote_copy(
                    src_ref=orecv.at[idx], dst_ref=orecv.at[idx],
                    send_sem=os_sems.at[0], recv_sem=or_sems.at[idx],
                    device_id=(me,), device_id_type=pl.DeviceIdType.MESH,
                ).wait_recv()
                acc = acc + orecv[idx].astype(f32)
            oacc[b] = acc
            pltpu.make_async_copy(oacc.at[b], out_hbm.at[b], st_sems.at[b]).start()


        def chunk_body(c, carry):
            col = pl.multiple_of(c * CW, CW)
            ts = []
            for i in range(3):
                pltpu.make_async_copy(
                    w_hbms[i].at[:, pl.ds(col, CW)],
                    w32.at[i, :, pl.ds(col, CW)],
                    ld_sems.at[2 + i * (D // CW) + c]).wait()
                wj = w32[i, :, pl.ds(col, CW)].astype(bf16)
                wqkv[:, pl.ds(i * D + col, CW)] = wj
                ts.append(jnp.dot(xg[0], wj, preferred_element_type=f32))
            cs = []
            for u in range(CW // DH):
                sl = slice(u * DH, (u + 1) * DH)
                q = rope(ts[0][:, sl], tab[0], tab[1]).astype(bf16)
                k = rope(ts[1][:, sl], tab[2], tab[3]).astype(bf16)
                v = ts[2][:, sl].astype(bf16)
                cs.append(attn_head(q, k, v))
            pltpu.make_async_copy(
                wo_hbm.at[pl.ds(col, CW), :],
                w32.at[3, pl.ds(col, CW), :],
                ld_sems.at[2 + NCH + c]).wait()
            woc = w32[3, pl.ds(col, CW), :].astype(bf16)
            wo[pl.ds(col, CW), :] = woc
            oacc[0] += jnp.dot(jnp.concatenate(cs, axis=1), woc,
                               preferred_element_type=f32)
            return carry

        oacc[0] = jnp.zeros((SQ, D), f32)
        lax.fori_loop(0, D // CW, chunk_body, 0)

        x_load(1).wait()
        xg[1] = xin[1].astype(bf16)
        x_send(2, 0).start()
        x_send(2, 1).start()

        def step(s, carry):
            b = (s >= 4).astype(jnp.int32)
            r = jnp.where((s == 1) | (s == 5), 1,
                          jnp.where((s == 2) | (s == 6), 3,
                                    jnp.where((s == 3) | (s == 4), 2, 0)))
            slot = r * 2 + b

            @pl.when(r > 0)
            def _():
                pltpu.make_async_remote_copy(
                    src_ref=xg.at[slot], dst_ref=xg.at[slot],
                    send_sem=xs_sems.at[0],
                    recv_sem=xr_sems.at[(r - 1) * 2 + b],
                    device_id=(me,), device_id_type=pl.DeviceIdType.MESH,
                ).wait_recv()

            part = compute(slot)

            @pl.when(s == 7)
            def _():
                finalize(1, part)

            @pl.when(r > 0)
            def _():
                osend[(r - 1) * 2 + b] = part.astype(bf16)
                o_copy(r, b).start()

            @pl.when(s == 1)
            def _():
                x_send(1, 1).start()
                x_send(3, 1).start()

            @pl.when(s == 6)
            def _():
                finalize(0, oacc[0])

            return carry

        lax.fori_loop(1, 8, step, 0)

        for b in range(B_LOC):
            pltpu.make_async_copy(oacc.at[b], out_hbm.at[b], st_sems.at[b]).wait()
        for d in range(1, N_DEV):
            for b in range(B_LOC):
                x_send(d, b).wait_send()
                o_copy(d, b).wait_send()

    out_shape = jax.ShapeDtypeStruct((B_LOC, SQ, D), jnp.float32)
    any_spec = pl.BlockSpec(memory_space=pl.ANY)
    return pl.pallas_call(
        body,
        out_shape=out_shape,
        in_specs=[any_spec] * 5,
        out_specs=any_spec,
        scratch_shapes=[
            pltpu.VMEM((B_LOC, SQ, D), f32),
            pltpu.VMEM((4, D, D), f32),
            pltpu.VMEM((D, 3 * D), bf16),
            pltpu.VMEM((D, D), bf16),
            pltpu.VMEM((8, SQ, D), bf16),
            pltpu.VMEM((6, SQ, D), bf16),
            pltpu.VMEM((6, SQ, D), bf16),
            pltpu.VMEM((B_LOC, SQ, D), f32),
            pltpu.VMEM((SQ, D), bf16),
            pltpu.VMEM((4, SQ, DH), f32),
            pltpu.SemaphoreType.DMA((18,)),
            pltpu.SemaphoreType.DMA((2,)),
            pltpu.SemaphoreType.DMA((6,)),
            pltpu.SemaphoreType.DMA((6,)),
            pltpu.SemaphoreType.DMA((6,)),
            pltpu.SemaphoreType.DMA((6,)),
        ],
        compiler_params=pltpu.CompilerParams(
            vmem_limit_bytes=100 * 1024 * 1024,
        ),
    )(x, Wq, Wk, Wv, Wo)
```
